```python
import numpy as np

kernel_name = "dist_max_ax1_xy_m4096_n1024"

def setup_inputs():
    return {"x": np.random.randn(8192, 2048).astype(np.float32)}

def reference(x: np.ndarray) -> np.ndarray:
    return np.max(x, axis=1, keepdims=True)
```

```python
import jax
import jax.numpy as jnp
from jax import lax
from jax.experimental import pallas as pl
from jax.experimental.pallas import tpu as pltpu

M, N = 4096, 1024
HALF = M // 2
MESH = pl.DeviceIdType.MESH
B = 128
NB = HALF // B
NEG = float("-inf")


def make(K=192, GS=12, seq=(256, 128), tail=(96, 32), ya=0, pre=6, altprio=False):
    assert B <= K < 2 * B and K % 8 == 0
    KR = K - B
    assert GS * B + sum(seq) + B == HALF and sum(tail) == B
    nseq, nt = len(seq), len(tail)

    def lanefold(ref, r0, rows):
        v = [ref[pl.ds(r0, rows), k * 128:(k + 1) * 128] for k in range(N // 128)]
        while len(v) > 1:
            v = [jnp.maximum(v[i], v[i + 1]) for i in range(0, len(v), 2)]
        return v[0]

    def blockmax(ref):
        return jnp.max(lanefold(ref, 0, B).T, axis=0, keepdims=True)

    def body(x_hbm, o_ref, xbuf, psend, precv, load_sems, ssems, rsems):
        my_x = lax.axis_index("x")
        my_y = lax.axis_index("y")
        py = (my_x, 1 - my_y)
        first = my_y
        second = 1 - my_y

        def rcopy(i, src, dst, dev):
            return pltpu.make_async_remote_copy(src_ref=src, dst_ref=dst, send_sem=ssems.at[i], recv_sem=rsems.at[i],
                                                device_id=dev, device_id_type=MESH)

        def ld(hh, h, g0, ng, r0, nr, sem):
            return pltpu.make_async_copy(x_hbm.at[hh, pl.ds(g0, ng), pl.ds(r0, nr), :],
                                         xbuf.at[h, pl.ds(g0, ng), pl.ds(r0, nr), :], load_sems.at[sem])

        ldF = []
        for j in range(B // 8):
            g0 = 2 if 8 * j < KR else 1
            ldF.append(ld(first, 0, g0, NB - g0, 8 * j, 8, 0))
        ldS = [ld(second, 1, 0, GS, 8 * j, 8, 1) for j in range(B // 8)]
        ldq = []
        g = GS
        for i, n in enumerate(seq):
            ldq.append((ld(second, 1, g, n // B, 0, B, 2 + i), g, n // B))
            g += n // B
        ldt = []
        r = 0
        for i, n in enumerate(tail):
            ldt.append((ld(second, 1, NB - 1, 1, r, n, 2 + nseq + i), r, n))
            r += n

        ldF[0].start()
        barrier = pltpu.get_barrier_semaphore()
        pl.semaphore_signal(barrier, inc=1, device_id=py, device_id_type=MESH)
        for cp in ldF[1:pre]:
            cp.start()
        raw0 = rcopy(0, x_hbm.at[first, 0], xbuf.at[0, 0], py)
        raws = [raw0]
        if KR:
            raws.append(rcopy(1, x_hbm.at[first, 1, pl.ds(0, KR), :], xbuf.at[0, 1, pl.ds(0, KR), :], py))
        pl.semaphore_wait(barrier, 1)
        for rw in raws:
            rw.start()
        for cp in ldF[pre:] + ldS:
            cp.start()
        for i, cp in enumerate([c for c, _, _ in ldq] + [c for c, _, _ in ldt]):
            cp.start()

        lane = lax.broadcasted_iota(jnp.int32, (8, B), 1)
        sub = lax.broadcasted_iota(jnp.int32, (8, B), 0)
        diag = lane - sub

        def xl_acc(acc, ref, r0, nrows):
            for j in range(nrows // 8):
                rm = jnp.max(lanefold(ref, r0 + 8 * j, 8), axis=1, keepdims=True)
                acc = jnp.where(diag == (r0 + 8 * j), rm, acc)
            return acc

        for cp in ldF:
            cp.wait()
        if KR:
            acc = xl_acc(jnp.full((8, B), NEG, jnp.float32), xbuf.at[0, 1], KR, B - KR)
            psend[:, pl.ds(B, B)] = jnp.max(acc, axis=0, keepdims=True)
        else:
            psend[:, pl.ds(B, B)] = blockmax(xbuf.at[0, 1])
        for g in range(2, NB):
            psend[:, pl.ds(g * B, B)] = blockmax(xbuf.at[0, g])
        prd = rcopy(2, psend.at[:, pl.ds(B, HALF - B)], precv.at[:, pl.ds(B, HALF - B)], py)
        prd.start()

        def fin_copy(i, lo, n, half):
            return rcopy(3 + i, o_ref.at[half, :, pl.ds(lo, n)], o_ref.at[half, :, pl.ds(lo, n)], py)

        def combine(nblk):
            prd.wait_recv()
            for rw in raws:
                rw.wait_recv()
            precv[:, pl.ds(0, B)] = blockmax(xbuf.at[0, 0])
            if KR:
                acc = xl_acc(jnp.broadcast_to(precv[:, pl.ds(B, B)], (8, B)), xbuf.at[0, 1], 0, KR)
                precv[:, pl.ds(B, B)] = jnp.max(acc, axis=0, keepdims=True)
            m = nblk * B
            o_ref[second, :, pl.ds(0, m)] = jnp.maximum(o_ref[second, :, pl.ds(0, m)], precv[:, pl.ds(0, m)])

        for cp in ldS:
            cp.wait()
        for g in range(GS):
            o_ref[second, :, pl.ds(g * B, B)] = blockmax(xbuf.at[1, g])
        if ya < 0:
            combine(GS)
        for c, (cp, g0, ng) in enumerate(ldq):
            cp.wait()
            for g in range(g0, g0 + ng):
                v = blockmax(xbuf.at[1, g])
                if c > ya:
                    v = jnp.maximum(v, precv[:, pl.ds(g * B, B)])
                o_ref[second, :, pl.ds(g * B, B)] = v
            if c == ya:
                combine(g0 + ng)
        f0 = fin_copy(0, 0, HALF - B, second)
        f0.start()
        prd.wait_send()
        for rw in raws:
            rw.wait_send()

        acc = jnp.broadcast_to(precv[:, pl.ds(HALF - B, B)], (8, B))
        for cp, r0, n in ldt:
            cp.wait()
            acc = xl_acc(acc, xbuf.at[1, NB - 1], r0, n)
        o_ref[second, :, pl.ds(HALF - B, B)] = jnp.max(acc, axis=0, keepdims=True)
        f1 = fin_copy(1, HALF - B, B, second)
        f1.start()

        f0.wait_send()
        fin_copy(0, 0, HALF - B, first).wait_recv()
        f1.wait_send()
        fin_copy(1, HALF - B, B, first).wait_recv()

    def fn(x):
        out = pl.pallas_call(
            body,
            out_shape=jax.ShapeDtypeStruct((2, 1, HALF), jnp.float32),
            in_specs=[pl.BlockSpec(memory_space=pl.ANY)],
            out_specs=pl.BlockSpec(memory_space=pltpu.VMEM),
            scratch_shapes=[
                pltpu.VMEM((2, NB, B, N), jnp.float32),
                pltpu.VMEM((1, HALF), jnp.float32),
                pltpu.VMEM((1, HALF), jnp.float32),
                pltpu.SemaphoreType.DMA((2 + nseq + nt,)),
                pltpu.SemaphoreType.DMA((5,)),
                pltpu.SemaphoreType.DMA((5,)),
            ],
            compiler_params=pltpu.CompilerParams(collective_id=0, vmem_limit_bytes=64 * 1024 * 1024,
                                                 disable_bounds_checks=True, disable_semaphore_checks=True),
        )(x.reshape(2, NB, B, N))
        return out.reshape(M, 1)
    return fn


_FN = make(K=208)


def pallas_dist_max_ax1_xy_m4096_n1024_kernel(x: jax.Array):
    return _FN(x)
```

```python
import jax
import jax.numpy as jnp
from jax import lax
from jax.experimental import pallas as pl
from jax.experimental.pallas import tpu as pltpu

M, N = 4096, 1024
B = 128
NB = M // (2 * B)
LAST = NB - 1
SUB = 8
LANES = 128

RAW_HEAD = 64
RAW_TAIL = 24
WIDE = 14
TAIL = (96, 32)
PRE = 6

NEG = float("-inf")
MESH = pl.DeviceIdType.MESH

RC_RAW0, RC_RAW1, RC_RAWT, RC_PART, RC_FIN0, RC_FIN1 = range(6)


def _lanefold(ref, r0, rows):
    v = [ref[pl.ds(r0, rows), k * LANES:(k + 1) * LANES] for k in range(N // LANES)]
    while len(v) > 1:
        v = [jnp.maximum(v[i], v[i + 1]) for i in range(0, len(v), 2)]
    return v[0]


def _blockmax(ref):
    return jnp.max(_lanefold(ref, 0, B).T, axis=0, keepdims=True)


def _body(x_hbm, o_ref, xbuf, rawbuf, psend, precv, load_sems, send_sems, recv_sems):
    my_x = lax.axis_index("x")
    my_y = lax.axis_index("y")
    peer = (my_x, 1 - my_y)
    first = my_y
    second = 1 - my_y

    def load(par, slot, g0, ng, r0, nr, sem):
        return pltpu.make_async_copy(
            x_hbm.at[pl.ds(g0, ng), par, pl.ds(r0, nr), :],
            xbuf.at[slot, pl.ds(g0, ng), pl.ds(r0, nr), :],
            load_sems.at[sem])

    def rcopy(i, src, dst):
        return pltpu.make_async_remote_copy(
            src_ref=src, dst_ref=dst,
            send_sem=send_sems.at[i], recv_sem=recv_sems.at[i],
            device_id=peer, device_id_type=MESH)

    def fin_copy(i, g0, ng, par):
        rows = o_ref.at[pl.ds(g0, ng), par]
        return rcopy(i, rows, rows)

    ld_first = []
    for r in range(0, B, SUB):
        g0 = 2 if r < RAW_HEAD else 1
        g1 = LAST if r >= B - RAW_TAIL else NB
        ld_first.append(load(first, 0, g0, g1 - g0, r, SUB, 0))
    ld_wide = [load(second, 1, 0, WIDE, r, SUB, 1) for r in range(0, B, SUB)]
    ld_mid = load(second, 1, WIDE, LAST - WIDE, 0, B, 2)
    ld_tail = []
    r = 0
    for i, n in enumerate(TAIL):
        ld_tail.append((load(second, 1, LAST, 1, r, n, 3 + i), r, n))
        r += n

    raw0 = rcopy(RC_RAW0, x_hbm.at[0, first], rawbuf.at[0])
    raw1 = rcopy(RC_RAW1, x_hbm.at[1, first, pl.ds(0, RAW_HEAD), :],
                 rawbuf.at[1, pl.ds(0, RAW_HEAD), :])
    rawt = rcopy(RC_RAWT, x_hbm.at[LAST, first, pl.ds(B - RAW_TAIL, RAW_TAIL), :],
                 rawbuf.at[1, pl.ds(B - RAW_TAIL, RAW_TAIL), :])
    part = rcopy(RC_PART, psend.at[pl.ds(1, NB - 1)], precv.at[pl.ds(1, NB - 1)])

    ld_first[0].start()
    barrier = pltpu.get_barrier_semaphore()
    pl.semaphore_signal(barrier, inc=1, device_id=peer, device_id_type=MESH)
    for cp in ld_first[1:PRE]:
        cp.start()
    pl.semaphore_wait(barrier, 1)
    raw0.start()
    raw1.start()
    for cp in ld_first[PRE:] + ld_wide:
        cp.start()

    lane = lax.broadcasted_iota(jnp.int32, (SUB, B), 1)
    sub = lax.broadcasted_iota(jnp.int32, (SUB, B), 0)
    diag = lane - sub

    def scatter_rows(acc, ref, r0, nrows, extra=None):
        for r in range(r0, r0 + nrows, SUB):
            m = _lanefold(ref, r, SUB)
            if extra is not None and r in extra:
                m = jnp.maximum(m, extra[r])
            acc = jnp.where(diag == r, jnp.max(m, axis=1, keepdims=True), acc)
        return acc

    def partmax(ref, r0, nrows, init):
        acc = scatter_rows(jnp.broadcast_to(init, (SUB, B)), ref, r0, nrows)
        return jnp.max(acc, axis=0, keepdims=True)

    for cp in ld_first:
        cp.wait()
    neg = jnp.full((1, B), NEG, jnp.float32)
    psend[1] = partmax(xbuf.at[0, 1], RAW_HEAD, B - RAW_HEAD, neg)
    for g in range(2, LAST):
        psend[g] = _blockmax(xbuf.at[0, g])
    psend[LAST] = partmax(xbuf.at[0, LAST], 0, B - RAW_TAIL, neg)
    part.start()
    rawt.start()
    ld_mid.start()
    for cp, _, _ in ld_tail:
        cp.start()

    raw0.wait_recv()
    precv[0] = _blockmax(rawbuf.at[0])
    raw1.wait_recv()
    part.wait_recv()
    precv[1] = partmax(rawbuf.at[1], 0, RAW_HEAD, precv[1])

    for cp in ld_wide:
        cp.wait()
    for g in range(WIDE):
        o_ref[g, second] = jnp.maximum(_blockmax(xbuf.at[1, g]), precv[g])
    ld_mid.wait()
    for g in range(WIDE, LAST):
        o_ref[g, second] = jnp.maximum(_blockmax(xbuf.at[1, g]), precv[g])
    fin_copy(RC_FIN0, 0, LAST, second).start()

    acc = jnp.broadcast_to(precv[LAST], (SUB, B))
    for i, (cp, r0, n) in enumerate(ld_tail):
        extra = None
        if i == len(TAIL) - 1:
            rawt.wait_recv()
            extra = {r: _lanefold(rawbuf.at[1], r, SUB)
                     for r in range(B - RAW_TAIL, B, SUB)}
        cp.wait()
        acc = scatter_rows(acc, xbuf.at[1, LAST], r0, n, extra)
    o_ref[LAST, second] = jnp.max(acc, axis=0, keepdims=True)
    fin_copy(RC_FIN1, LAST, 1, second).start()

    for cp in (raw0, raw1, part, rawt):
        cp.wait_send()
    fin_copy(RC_FIN0, 0, LAST, second).wait_send()
    fin_copy(RC_FIN0, 0, LAST, first).wait_recv()
    fin_copy(RC_FIN1, LAST, 1, second).wait_send()
    fin_copy(RC_FIN1, LAST, 1, first).wait_recv()


def pallas_dist_max_ax1_xy_m4096_n1024_kernel(
x: jax.Array,
):
    out = pl.pallas_call(
        _body,
        out_shape=jax.ShapeDtypeStruct((NB, 2, 1, B), jnp.float32),
        in_specs=[pl.BlockSpec(memory_space=pl.ANY)],
        out_specs=pl.BlockSpec(memory_space=pltpu.VMEM),
        scratch_shapes=[
            pltpu.VMEM((2, NB, B, N), jnp.float32),
            pltpu.VMEM((2, B, N), jnp.float32),
            pltpu.VMEM((NB, 1, B), jnp.float32),
            pltpu.VMEM((NB, 1, B), jnp.float32),
            pltpu.SemaphoreType.DMA((3 + len(TAIL),)),
            pltpu.SemaphoreType.DMA((6,)),
            pltpu.SemaphoreType.DMA((6,)),
        ],
        compiler_params=pltpu.CompilerParams(
            collective_id=0,
            vmem_limit_bytes=64 * 1024 * 1024,
            disable_bounds_checks=True,
            disable_semaphore_checks=True,
        ),
    )(x.reshape(NB, 2, B, N))
    return out.reshape(M, 1)
```

```python
import jax
import jax.numpy as jnp
from jax import lax
from jax.experimental import pallas as pl
from jax.experimental.pallas import tpu as pltpu

M, N = 4096, 1024
B = 128
NB = M // (2 * B)
LAST = NB - 1
SUB, LANES = 8, 128
KT = N // LANES
NT = (B // SUB) * KT

DUP = 96
HEAD = 95
WIDE = 13
TAIL = (96, 32)
PRE = 6


def _pieces(step):
    cuts = [0] + list(range(7, NT - 8, step)) + [NT]
    return list(zip(cuts[:-1], cuts[1:]))


FINE = _pieces(8)
COARSE = _pieces(16)

NEG = float("-inf")
MESH = pl.DeviceIdType.MESH

RC_RAW0, RC_RAW1, RC_RAWD, RC_PART, RC_DPART, RC_FIN0, RC_FIN1 = range(7)
N_RC = 7


def _fold(ref, lo, hi):
    v = [ref[t] for t in range(lo, hi)]
    while len(v) > 1:
        v = [jnp.maximum(v[i], v[i + 1]) if i + 1 < len(v) else v[i]
             for i in range(0, len(v), 2)]
    return v[0]


def _blockmax(ref):
    m = jnp.max(ref[...].reshape(B // SUB, KT, SUB, LANES), axis=1).reshape(B, LANES)
    return jnp.max(m.T, axis=0, keepdims=True)


def _body(x_hbm, o_ref, xbuf, rawbuf, psend, precv, dsend, drecv,
          load_sems, send_sems, recv_sems):
    my_x = lax.axis_index("x")
    my_y = lax.axis_index("y")
    peer = (my_x, 1 - my_y)
    first = my_y
    second = 1 - my_y

    def load(par, slot, g0, ng, lo, hi, sem):
        return pltpu.make_async_copy(
            x_hbm.at[pl.ds(g0, ng), par, pl.ds(lo, hi - lo)],
            xbuf.at[slot, pl.ds(g0, ng), pl.ds(lo, hi - lo)],
            load_sems.at[sem])

    def rcopy(i, src, dst):
        return pltpu.make_async_remote_copy(
            src_ref=src, dst_ref=dst,
            send_sem=send_sems.at[i], recv_sem=recv_sems.at[i],
            device_id=peer, device_id_type=MESH)

    def raw_copy(i, g, lo, hi):
        return rcopy(i, x_hbm.at[g, first, pl.ds(lo, hi - lo)],
                     rawbuf.at[g, pl.ds(lo, hi - lo)])

    def fin_copy(i, g0, ng, par):
        rows = o_ref.at[pl.ds(g0, ng), par]
        return rcopy(i, rows, rows)

    ld_first = []
    for lo, hi in FINE:
        g0 = 2 if lo < HEAD else 1
        ld_first.append(load(first, 0, g0, NB - g0, lo, hi, 0))
    ld_wide = [load(second, 1, 0, WIDE, lo, hi, 1) for lo, hi in FINE]
    ld_mid = [load(second, 1, WIDE, LAST - WIDE, lo, hi, 2) for lo, hi in COARSE]
    ld_tail = []
    lo = 0
    for i, n in enumerate(TAIL):
        ld_tail.append((load(second, 1, LAST, 1, lo, lo + n, 3 + i), lo, lo + n))
        lo += n
    ld_dup = load(first, 0, 0, 1, DUP, NT, 3 + len(TAIL))

    raw0 = raw_copy(RC_RAW0, 0, 0, DUP)
    raw1 = raw_copy(RC_RAW1, 1, 0, HEAD)
    rawd = raw_copy(RC_RAWD, 0, DUP, NT)
    part = rcopy(RC_PART, psend.at[pl.ds(1, NB - 1)], precv.at[pl.ds(1, NB - 1)])
    dpart = rcopy(RC_DPART, dsend, drecv)

    ld_first[0].start()
    barrier = pltpu.get_barrier_semaphore()
    pl.semaphore_signal(barrier, inc=1, device_id=peer, device_id_type=MESH)
    for cp in ld_first[1:PRE]:
        cp.start()
    pl.semaphore_wait(barrier, 1)
    raw0.start()
    raw1.start()
    for cp in ld_first[PRE:] + ld_wide:
        cp.start()

    lane = lax.broadcasted_iota(jnp.int32, (SUB, B), 1)
    sub = lax.broadcasted_iota(jnp.int32, (SUB, B), 0)
    diag = lane - sub

    def scatter_rows(acc, ref, lo, hi):
        for q in range(lo // KT, (hi - 1) // KT + 1):
            m = _fold(ref, max(lo, q * KT), min(hi, (q + 1) * KT))
            acc = jnp.where(diag == q * SUB, jnp.max(m, axis=1, keepdims=True), acc)
        return acc

    def partmax(ref, lo, hi, init):
        acc = scatter_rows(jnp.broadcast_to(init, (SUB, B)), ref, lo, hi)
        return jnp.max(acc, axis=0, keepdims=True)

    for cp in ld_first:
        cp.wait()
    neg = jnp.full((1, B), NEG, jnp.float32)
    psend[1] = partmax(xbuf.at[0, 1], HEAD, NT, neg)
    for g in range(2, NB):
        psend[g] = _blockmax(xbuf.at[0, g])
    part.start()
    rawd.start()
    for cp in ld_mid:
        cp.start()
    for cp, _, _ in ld_tail:
        cp.start()
    ld_dup.start()

    raw0.wait_recv()
    precv[0] = partmax(rawbuf.at[0], 0, DUP, neg)
    raw1.wait_recv()
    part.wait_recv()
    precv[1] = partmax(rawbuf.at[1], 0, HEAD, precv[1])

    for cp in ld_wide:
        cp.wait()
    dsend[...] = jnp.maximum(_blockmax(xbuf.at[1, 0]), precv[0])
    for g in range(1, WIDE):
        o_ref[g, second] = jnp.maximum(_blockmax(xbuf.at[1, g]), precv[g])
    for cp in ld_mid:
        cp.wait()
    for g in range(WIDE, LAST):
        o_ref[g, second] = jnp.maximum(_blockmax(xbuf.at[1, g]), precv[g])
    dpart.start()
    fin_copy(RC_FIN0, 1, LAST - 1, second).start()

    acc = jnp.broadcast_to(precv[LAST], (SUB, B))
    for cp, lo, hi in ld_tail:
        cp.wait()
        acc = scatter_rows(acc, xbuf.at[1, LAST], lo, hi)
    o_ref[LAST, second] = jnp.max(acc, axis=0, keepdims=True)
    fin_copy(RC_FIN1, LAST, 1, second).start()

    ld_dup.wait()
    mine = partmax(xbuf.at[0, 0], DUP, NT, neg)
    rawd.wait_recv()
    o_ref[0, second] = partmax(rawbuf.at[0], DUP, NT, dsend[...])
    dpart.wait_recv()
    o_ref[0, first] = jnp.maximum(mine, drecv[...])

    for cp in (raw0, raw1, part, rawd, dpart):
        cp.wait_send()
    fin_copy(RC_FIN0, 1, LAST - 1, second).wait_send()
    fin_copy(RC_FIN0, 1, LAST - 1, first).wait_recv()
    fin_copy(RC_FIN1, LAST, 1, second).wait_send()
    fin_copy(RC_FIN1, LAST, 1, first).wait_recv()


def pallas_dist_max_ax1_xy_m4096_n1024_kernel(
x: jax.Array,
):
    tiles = (x.reshape(M // SUB, SUB, KT, LANES)
             .transpose(0, 2, 1, 3)
             .reshape(NB, 2, NT, SUB, LANES))
    out = pl.pallas_call(
        _body,
        out_shape=jax.ShapeDtypeStruct((NB, 2, 1, B), jnp.float32),
        in_specs=[pl.BlockSpec(memory_space=pl.ANY)],
        out_specs=pl.BlockSpec(memory_space=pltpu.VMEM),
        scratch_shapes=[
            pltpu.VMEM((2, NB, NT, SUB, LANES), jnp.float32),
            pltpu.VMEM((2, NT, SUB, LANES), jnp.float32),
            pltpu.VMEM((NB, 1, B), jnp.float32),
            pltpu.VMEM((NB, 1, B), jnp.float32),
            pltpu.VMEM((1, B), jnp.float32),
            pltpu.VMEM((1, B), jnp.float32),
            pltpu.SemaphoreType.DMA((4 + len(TAIL),)),
            pltpu.SemaphoreType.DMA((N_RC,)),
            pltpu.SemaphoreType.DMA((N_RC,)),
        ],
        compiler_params=pltpu.CompilerParams(
            collective_id=0,
            vmem_limit_bytes=64 * 1024 * 1024,
            disable_bounds_checks=True,
            disable_semaphore_checks=True,
        ),
    )(tiles)
    return out.reshape(M, 1)
```

```python
import jax
import jax.numpy as jnp
from jax import lax
from jax.experimental import pallas as pl
from jax.experimental.pallas import tpu as pltpu

M, N = 4096, 1024
B = 128
NB = M // (2 * B)
LAST = NB - 1
SUB, LANES = 8, 128
KT = N // LANES
NT = (B // SUB) * KT

DUP = 96
HEAD = 96
WIDE = 13
TAIL = (96, 32)
PRE = 6


def _pieces(step):
    cuts = [0] + list(range(7, NT - 8, step)) + [NT]
    return list(zip(cuts[:-1], cuts[1:]))


FINE = _pieces(8)
COARSE = _pieces(16)

NEG = float("-inf")
MESH = pl.DeviceIdType.MESH

RC_RAW0, RC_RAW1, RC_RAWD, RC_PART, RC_DPART, RC_FIN0, RC_FIN1 = range(7)
N_RC = 7


def _fold(ref, lo, hi):
    v = [ref[t] for t in range(lo, hi)]
    while len(v) > 1:
        v = [jnp.maximum(v[i], v[i + 1]) if i + 1 < len(v) else v[i]
             for i in range(0, len(v), 2)]
    return v[0]


def _blockmax(ref):
    m = jnp.max(ref[...].reshape(B // SUB, KT, SUB, LANES), axis=1).reshape(B, LANES)
    return jnp.max(m.T, axis=0, keepdims=True)


def _body(x_hbm, o_ref, xbuf, rawbuf, sbuf, psend, precv, dsend, drecv,
          load_sems, bounce_sems, send_sems, recv_sems):
    my_x = lax.axis_index("x")
    my_y = lax.axis_index("y")
    peer = (my_x, 1 - my_y)
    first = my_y
    second = 1 - my_y

    def load(par, slot, g0, ng, lo, hi, sem):
        return pltpu.make_async_copy(
            x_hbm.at[pl.ds(g0, ng), par, pl.ds(lo, hi - lo)],
            xbuf.at[slot, pl.ds(g0, ng), pl.ds(lo, hi - lo)],
            load_sems.at[sem])

    def rcopy(i, src, dst):
        return pltpu.make_async_remote_copy(
            src_ref=src, dst_ref=dst,
            send_sem=send_sems.at[i], recv_sem=recv_sems.at[i],
            device_id=peer, device_id_type=MESH)

    def raw_copy(i, g, lo, hi):
        return rcopy(i, x_hbm.at[g, first, pl.ds(lo, hi - lo)],
                     rawbuf.at[g, pl.ds(lo, hi - lo)])

    def fin_copy(i, g0, ng, par):
        rows = o_ref.at[pl.ds(g0, ng), par]
        return rcopy(i, rows, rows)

    ld_first = [load(first, 0, 2, NB - 2, lo, hi, 0) for lo, hi in FINE]
    ld_wide = [load(second, 1, 0, WIDE, lo, hi, 1) for lo, hi in FINE]
    ld_mid = [load(second, 1, WIDE, LAST - WIDE, lo, hi, 2) for lo, hi in COARSE]
    ld_tail = []
    lo = 0
    for i, n in enumerate(TAIL):
        ld_tail.append((load(second, 1, LAST, 1, lo, lo + n, 3 + i), lo, lo + n))
        lo += n
    ld_dup = load(first, 0, 0, 1, DUP, NT, 3 + len(TAIL))
    bounce_in = pltpu.make_async_copy(
        x_hbm.at[1, first, pl.ds(HEAD, NT - HEAD)], sbuf, bounce_sems.at[0])
    bounce_out = pltpu.make_async_copy(
        sbuf, xbuf.at[0, 1, pl.ds(HEAD, NT - HEAD)], bounce_sems.at[1])

    raw0 = raw_copy(RC_RAW0, 0, 0, DUP)
    raw1 = raw_copy(RC_RAW1, 1, 0, HEAD)
    rawd = raw_copy(RC_RAWD, 0, DUP, NT)
    part = rcopy(RC_PART, psend.at[pl.ds(1, NB - 1)], precv.at[pl.ds(1, NB - 1)])
    dpart = rcopy(RC_DPART, dsend, drecv)

    ld_first[0].start()
    bounce_in.start()
    barrier = pltpu.get_barrier_semaphore()
    pl.semaphore_signal(barrier, inc=1, device_id=peer, device_id_type=MESH)
    for cp in ld_first[1:PRE]:
        cp.start()
    pl.semaphore_wait(barrier, 1)
    raw0.start()
    raw1.start()
    for cp in ld_first[PRE:] + ld_wide:
        cp.start()

    lane = lax.broadcasted_iota(jnp.int32, (SUB, B), 1)
    sub = lax.broadcasted_iota(jnp.int32, (SUB, B), 0)
    diag = lane - sub

    def scatter_rows(acc, ref, lo, hi):
        for q in range(lo // KT, (hi - 1) // KT + 1):
            m = _fold(ref, max(lo, q * KT), min(hi, (q + 1) * KT))
            acc = jnp.where(diag == q * SUB, jnp.max(m, axis=1, keepdims=True), acc)
        return acc

    def partmax(ref, lo, hi, init):
        acc = scatter_rows(jnp.broadcast_to(init, (SUB, B)), ref, lo, hi)
        return jnp.max(acc, axis=0, keepdims=True)

    bounce_in.wait()
    bounce_out.start()
    bounce_out.wait()
    for cp in ld_first:
        cp.wait()
    neg = jnp.full((1, B), NEG, jnp.float32)
    psend[1] = partmax(xbuf.at[0, 1], HEAD, NT, neg)
    for g in range(2, NB):
        psend[g] = _blockmax(xbuf.at[0, g])
    part.start()
    rawd.start()
    for cp in ld_mid:
        cp.start()
    for cp, _, _ in ld_tail:
        cp.start()
    ld_dup.start()

    raw0.wait_recv()
    precv[0] = partmax(rawbuf.at[0], 0, DUP, neg)
    raw1.wait_recv()
    part.wait_recv()
    precv[1] = partmax(rawbuf.at[1], 0, HEAD, precv[1])

    for cp in ld_wide:
        cp.wait()
    dsend[...] = jnp.maximum(_blockmax(xbuf.at[1, 0]), precv[0])
    for g in range(1, WIDE):
        o_ref[g, second] = jnp.maximum(_blockmax(xbuf.at[1, g]), precv[g])
    for cp in ld_mid:
        cp.wait()
    for g in range(WIDE, LAST):
        o_ref[g, second] = jnp.maximum(_blockmax(xbuf.at[1, g]), precv[g])
    dpart.start()
    fin_copy(RC_FIN0, 1, LAST - 1, second).start()

    acc = jnp.broadcast_to(precv[LAST], (SUB, B))
    for cp, lo, hi in ld_tail:
        cp.wait()
        acc = scatter_rows(acc, xbuf.at[1, LAST], lo, hi)
    o_ref[LAST, second] = jnp.max(acc, axis=0, keepdims=True)
    fin_copy(RC_FIN1, LAST, 1, second).start()

    ld_dup.wait()
    mine = partmax(xbuf.at[0, 0], DUP, NT, neg)
    rawd.wait_recv()
    o_ref[0, second] = partmax(rawbuf.at[0], DUP, NT, dsend[...])
    dpart.wait_recv()
    o_ref[0, first] = jnp.maximum(mine, drecv[...])

    for cp in (raw0, raw1, part, rawd, dpart):
        cp.wait_send()
    fin_copy(RC_FIN0, 1, LAST - 1, second).wait_send()
    fin_copy(RC_FIN0, 1, LAST - 1, first).wait_recv()
    fin_copy(RC_FIN1, LAST, 1, second).wait_send()
    fin_copy(RC_FIN1, LAST, 1, first).wait_recv()


def pallas_dist_max_ax1_xy_m4096_n1024_kernel(
x: jax.Array,
):
    tiles = (x.reshape(M // SUB, SUB, KT, LANES)
             .transpose(0, 2, 1, 3)
             .reshape(NB, 2, NT, SUB, LANES))
    out = pl.pallas_call(
        _body,
        out_shape=jax.ShapeDtypeStruct((NB, 2, 1, B), jnp.float32),
        in_specs=[pl.BlockSpec(memory_space=pl.ANY)],
        out_specs=pl.BlockSpec(memory_space=pltpu.VMEM),
        scratch_shapes=[
            pltpu.VMEM((2, NB, NT, SUB, LANES), jnp.float32),
            pltpu.VMEM((2, NT, SUB, LANES), jnp.float32),
            pltpu.SMEM((NT - HEAD, SUB, LANES), jnp.float32),
            pltpu.VMEM((NB, 1, B), jnp.float32),
            pltpu.VMEM((NB, 1, B), jnp.float32),
            pltpu.VMEM((1, B), jnp.float32),
            pltpu.VMEM((1, B), jnp.float32),
            pltpu.SemaphoreType.DMA((4 + len(TAIL),)),
            pltpu.SemaphoreType.DMA((2,)),
            pltpu.SemaphoreType.DMA((N_RC,)),
            pltpu.SemaphoreType.DMA((N_RC,)),
        ],
        compiler_params=pltpu.CompilerParams(
            collective_id=0,
            vmem_limit_bytes=64 * 1024 * 1024,
            disable_bounds_checks=True,
            disable_semaphore_checks=True,
        ),
    )(tiles)
    return out.reshape(M, 1)
```
